```python
import numpy as np

kernel_name = "dist_layernorm_xy_m6144_n2048"

def setup_inputs():
    x = np.random.randn(12288, 4096).astype(np.float32)
    gamma = np.random.randn(4096).astype(np.float32)
    beta = np.random.randn(4096).astype(np.float32)
    return {"x": x, "gamma": gamma, "beta": beta}

def reference(x: np.ndarray, gamma: np.ndarray, beta: np.ndarray) -> np.ndarray:
    eps = 1e-5
    mean = np.mean(x, axis=1, keepdims=True)
    var = np.var(x, axis=1, keepdims=True)
    return gamma * (x - mean) / np.sqrt(var + eps) + beta
```

```python
import jax
import jax.numpy as jnp
from jax import lax
from jax.experimental import pallas as pl
from jax.experimental.pallas import tpu as pltpu

_ROWS, _COLS = 6144, 2048
_EPS = 1e-5
_LANES, _SUB = 128, 8
_COL_TILES = _COLS // _LANES

_PIECES, _UNIT = 4, 128
_PIECE_ROWS = _ROWS // _PIECES

_BLOCK_ROWS = (512,) * 10 + (280, 384, 192, 96, 48, 24)
_DEFERRED = 5
_LOADS_IN_FLIGHT = 2
_HALF = _LANES // 2

_UNROLL_STATS, _UNROLL_UNPACK, _UNROLL_NORM = 8, 32, 4


def _layout():
    blocks, start = [], 0
    for rows in _BLOCK_ROWS:
        piece, offset = divmod(start, _PIECE_ROWS)
        assert rows % _SUB == 0 and rows <= _SUB * _HALF and offset + rows <= _PIECE_ROWS
        blocks.append((start, rows, piece, offset))
        start += rows
    assert start == _ROWS
    return tuple(blocks)


_BLOCKS = _layout()
_NB = len(_BLOCKS)


def _unroll_for(wanted, groups):
    u = min(wanted, groups)
    while groups % u:
        u -= 1
    return u


def _row_slice(start, n):
    return pl.ds(start if isinstance(start, int) else pl.multiple_of(start, _SUB), n)


def _repeat(n, body, carry, first=0):
    if n - first <= 0:
        return carry
    if n - first == 1:
        return body(first, carry)
    return lax.fori_loop(first, n, body, carry)


def _add_tiles(tiles):
    even, odd = tiles[0], tiles[1]
    for k in range(2, len(tiles), 2):
        even, odd = even + tiles[k], odd + tiles[k + 1]
    return even + odd


def _kernel(x_hbm, gamma_hbm, beta_hbm, *refs):
    outs = [o.reshape(_PIECE_ROWS, _COLS) for o in refs[:_PIECES]]
    (gb, gb8, sent, received, mean_b, rstd_b, load_sem, gb_sem, send_sem, recv_sem) = refs[_PIECES:]
    neighbour = (lax.axis_index("x"), 1 - lax.axis_index("y"))
    lane = lax.broadcasted_iota(jnp.int32, (_SUB, _LANES), 1)

    def load(i):
        start, rows, piece, offset = _BLOCKS[i]
        return pltpu.make_async_copy(
            x_hbm.at[pl.ds(start, rows)], outs[piece].at[pl.ds(offset, rows)], load_sem.at[i]
        )

    def exchange(i):
        return pltpu.make_async_remote_copy(
            src_ref=sent.at[i], dst_ref=received.at[i],
            send_sem=send_sem.at[i], recv_sem=recv_sem.at[i],
            device_id=neighbour, device_id_type=pl.DeviceIdType.MESH,
        )

    def reduce_rows(i, partial, collect, packed):
        groups = _BLOCKS[i][1] // _SUB
        unroll = _unroll_for(_UNROLL_STATS, groups)

        def partials(g0):
            return tuple(partial(g0 + u) for u in range(unroll))

        def finish(g0, parts, packed):
            for u in range(unroll):
                packed = collect(g0 + u, jnp.sum(parts[u], axis=1, keepdims=True), packed)
            return packed

        def step(t, carry):
            parts, packed = carry
            return partials(t * unroll), finish((t - 1) * unroll, parts, packed)

        carry = _repeat(groups // unroll, step, (partials(0), packed), first=1)
        return finish(groups - unroll, *carry)

    def local_stats(i):
        _, _, piece, offset = _BLOCKS[i]

        def tiles(g):
            rows = _row_slice(offset + g * _SUB, _SUB)
            return [outs[piece][rows, pl.ds(c * _LANES, _LANES)] for c in range(_COL_TILES)]

        def keep_mean(g, total, packed):
            mean = total * (1.0 / _COLS)
            mean_b[_row_slice(g * _SUB, _SUB), :] = jnp.broadcast_to(mean, (_SUB, _LANES))
            return jnp.where(lane == g, mean, packed)

        def centred_squares(g):
            mean = mean_b[_row_slice(g * _SUB, _SUB), :]
            deviations = [t - mean for t in tiles(g)]
            return _add_tiles([d * d for d in deviations])

        packed = reduce_rows(
            i, lambda g: _add_tiles(tiles(g)), keep_mean, jnp.zeros((_SUB, _LANES), jnp.float32)
        )
        return reduce_rows(
            i, centred_squares, lambda g, m2, packed: jnp.where(lane == g + _HALF, m2, packed), packed
        )

    def merge_stats(j):
        groups = _BLOCKS[j][1] // _SUB
        unroll = _unroll_for(_UNROLL_UNPACK, groups)
        mine, theirs = sent[j], received[j]
        both = mine + theirs
        gap = mine - theirs
        low = lane < _HALF
        means = jnp.where(low, both * 0.5, 0.0)
        m2_terms = jnp.where(low, gap * gap * (_COLS * 0.5), both)
        group_of_lane = lax.bitwise_and(lane, _HALF - 1)

        def step(t, carry):
            for u in range(unroll):
                g = t * unroll + u
                here = group_of_lane == g
                mean = jnp.sum(jnp.where(here, means, 0.0), axis=1, keepdims=True)
                m2 = jnp.sum(jnp.where(here, m2_terms, 0.0), axis=1, keepdims=True)
                rstd = 1.0 / jnp.sqrt(m2 * (1.0 / (2 * _COLS)) + _EPS)
                mean_b[_row_slice(g * _SUB, _SUB), :] = jnp.broadcast_to(mean, (_SUB, _LANES))
                rstd_b[_row_slice(g * _SUB, _SUB), :] = jnp.broadcast_to(rstd, (_SUB, _LANES))
            return carry

        _repeat(groups // unroll, step, 0)

    def normalise(j):
        _, rows, piece, offset = _BLOCKS[j]
        groups = rows // _SUB
        unroll = _unroll_for(_UNROLL_NORM, groups)
        slab = unroll * _SUB

        def step(t, carry):
            at = _row_slice(offset + t * slab, slab)
            x = outs[piece][at, :]
            mean = mean_b[_row_slice(t * slab, slab), :]
            rstd = rstd_b[_row_slice(t * slab, slab), :]
            ys = []
            for c in range(_COL_TILES):
                cols = slice(c * _LANES, (c + 1) * _LANES)
                gamma = jnp.tile(gb8[0, :, cols], (unroll, 1))
                beta = jnp.tile(gb8[1, :, cols], (unroll, 1))
                ys.append((x[:, cols] - mean) * rstd * gamma + beta)
            outs[piece][at, :] = jnp.concatenate(ys, axis=1)
            return carry

        _repeat(groups // unroll, step, 0)

    for i in range(_LOADS_IN_FLIGHT):
        load(i).start()
    gamma_copy = pltpu.make_async_copy(gamma_hbm, gb.at[pl.ds(0, 1)], gb_sem.at[0])
    beta_copy = pltpu.make_async_copy(beta_hbm, gb.at[pl.ds(1, 1)], gb_sem.at[1])
    gamma_copy.start()
    beta_copy.start()
    barrier = pltpu.get_barrier_semaphore()
    pl.semaphore_signal(barrier, inc=1, device_id=neighbour, device_id_type=pl.DeviceIdType.MESH)

    def front(i):
        load(i).wait()
        if i + _LOADS_IN_FLIGHT < _NB:
            load(i + _LOADS_IN_FLIGHT).start()
        sent[i] = local_stats(i)
        if i == 0:
            pl.semaphore_wait(barrier, 1)
        exchange(i).start()

    def back(j):
        if j == 0:
            gamma_copy.wait()
            beta_copy.wait()
            gb8[0] = jnp.broadcast_to(gb[0:1, :], (_SUB, _COLS))
            gb8[1] = jnp.broadcast_to(gb[1:2, :], (_SUB, _COLS))
        exchange(j).wait_recv()
        exchange(j).wait_send()
        merge_stats(j)
        normalise(j)

    done = 0
    for i in range(_NB):
        front(i)
        while done < min(i, _NB - _DEFERRED):
            back(done)
            done += 1
    while done < _NB:
        back(done)
        done += 1


def pallas_dist_layernorm_xy_m6144_n2048_kernel(x: jax.Array, gamma: jax.Array, beta: jax.Array):
    assert x.shape == (_ROWS, _COLS) and gamma.shape == beta.shape == (_COLS,)
    x, gamma, beta = (a.astype(jnp.float32) for a in (x, gamma, beta))
    max_rows = max(_BLOCK_ROWS)
    pieces = pl.pallas_call(
        _kernel,
        out_shape=[pltpu.VMEM((_PIECE_ROWS // _UNIT, _UNIT, _COLS), jnp.float32)] * _PIECES,
        in_specs=[pl.BlockSpec(memory_space=pl.ANY)] * 3,
        out_specs=[pl.BlockSpec(memory_space=pltpu.VMEM)] * _PIECES,
        scratch_shapes=[
            pltpu.VMEM((2, _COLS), jnp.float32),
            pltpu.VMEM((2, _SUB, _COLS), jnp.float32),
            pltpu.VMEM((_NB, _SUB, _LANES), jnp.float32),
            pltpu.VMEM((_NB, _SUB, _LANES), jnp.float32),
            pltpu.VMEM((max_rows, _LANES), jnp.float32),
            pltpu.VMEM((max_rows, _LANES), jnp.float32),
            pltpu.SemaphoreType.DMA((_NB,)),
            pltpu.SemaphoreType.DMA((2,)),
            pltpu.SemaphoreType.DMA((_NB,)),
            pltpu.SemaphoreType.DMA((_NB,)),
        ],
        compiler_params=pltpu.CompilerParams(vmem_limit_bytes=8 * 1024 * 1024, collective_id=0),
    )(x, gamma.reshape(1, _COLS), beta.reshape(1, _COLS))
    return jnp.concatenate(pieces, axis=0).reshape(_ROWS, _COLS)
```
